```python
import numpy as np

kernel_name = "dist_sum_ax1_xy_m512_n256"

def setup_inputs():
    return {"x": np.random.randn(1024, 512).astype(np.float32)}

def reference(x: np.ndarray) -> np.ndarray:
    return np.sum(x, axis=1, keepdims=True)
```

```python
import jax
import jax.numpy as jnp
from jax import lax
from jax.experimental import pallas as pl
from jax.experimental.pallas import tpu as pltpu

LANES = 128
SUBLANES = 8


def pallas_dist_sum_ax1_xy_m512_n256_kernel(x: jax.Array):
    m, n = x.shape
    n_blocks = m // LANES

    def body(x_hbm, o_ref, x_vmem, part, recv, load_sems, send_sems, recv_sems):
        loads = []
        for b in range(n_blocks):
            rows = pl.ds(b * LANES, LANES)
            load = pltpu.make_async_copy(x_hbm.at[rows], x_vmem.at[rows], load_sems.at[b])
            load.start()
            loads.append(load)

        peer = lax.axis_index("x") * 2 + (1 - lax.axis_index("y"))
        barrier = pltpu.get_barrier_semaphore()
        pl.semaphore_signal(barrier, 1, device_id=peer, device_id_type=pl.DeviceIdType.LOGICAL)

        sends = [
            pltpu.make_async_remote_copy(
                part.at[b], recv.at[b], send_sems.at[b], recv_sems.at[b],
                device_id=peer, device_id_type=pl.DeviceIdType.LOGICAL)
            for b in range(n_blocks)
        ]
        lane = lax.broadcasted_iota(jnp.int32, (SUBLANES, LANES), 1)
        sublane = lax.broadcasted_iota(jnp.int32, (SUBLANES, LANES), 0)
        mine = []
        for b in range(n_blocks):
            loads[b].wait()
            acc = jnp.zeros((SUBLANES, LANES), jnp.float32)
            for r in range(0, LANES, SUBLANES):
                rows = pl.ds(b * LANES + r, SUBLANES)
                s = x_vmem[rows, 0:LANES]
                for c in range(LANES, n, LANES):
                    s = s + x_vmem[rows, c:c + LANES]
                acc = jnp.where(lane - sublane == r, jnp.sum(s, axis=1, keepdims=True), acc)
            p = jnp.sum(acc, axis=0, keepdims=True)
            part[b] = p
            mine.append(p)
            if b == 0:
                pl.semaphore_wait(barrier, 1)
            sends[b].start()

        for b in range(n_blocks):
            if b == n_blocks - 1:
                for send in sends:
                    send.wait_send()
            sends[b].wait_recv()
            o_ref[pl.ds(b, 1)] = mine[b] + recv[b]

    out = pl.pallas_call(
        body,
        out_shape=jax.ShapeDtypeStruct((n_blocks, LANES), x.dtype),
        in_specs=[pl.BlockSpec(memory_space=pltpu.MemorySpace.HBM)],
        out_specs=pl.BlockSpec(memory_space=pltpu.VMEM),
        scratch_shapes=[
            pltpu.VMEM((m, n), jnp.float32),
            pltpu.VMEM((n_blocks, 1, LANES), jnp.float32),
            pltpu.VMEM((n_blocks, 1, LANES), jnp.float32),
            pltpu.SemaphoreType.DMA((n_blocks,)),
            pltpu.SemaphoreType.DMA((n_blocks,)),
            pltpu.SemaphoreType.DMA((n_blocks,)),
        ],
        compiler_params=pltpu.CompilerParams(
            collective_id=0, disable_bounds_checks=True, disable_semaphore_checks=True),
    )(x)
    return out.reshape(m, 1)
```

```python
import jax
import jax.numpy as jnp
from jax import lax
from jax.experimental import pallas as pl
from jax.experimental.pallas import tpu as pltpu

SUBLANES = 8
LANES = 128
SHARD_SHAPE = (512, 256)
N_BLOCKS = SHARD_SHAPE[0] // LANES
GROUPS_PER_BLOCK = LANES // SUBLANES

LEFT, RIGHT, BOTH = (0, LANES), (LANES, LANES), (0, 2 * LANES)

LOADS = (
    ((128, BOTH),),
    ((128, BOTH),),
    ((128, BOTH),),
    ((32, BOTH), (24, BOTH), (24, BOTH), (8, BOTH), (8, BOTH), (8, BOTH), (8, BOTH),
     (8, LEFT), (8, RIGHT), (8, LEFT), (8, RIGHT)),
)
LOAD_QUEUE = (0, 0, 1, 1)

MERGE_ORDER = (
    tuple(range(GROUPS_PER_BLOCK)),
    tuple(range(GROUPS_PER_BLOCK)),
    tuple(range(GROUPS_PER_BLOCK)),
    (10, 0, 1, 11, 2, 3, 12, 4, 5, 13, 6, 7, 14, 8, 9, 15),
)


def _kernel_body(x_hbm, out_ref, x_vmem, load_sems, send_sems, recv_sems, *messages):
    outbox, inbox = messages[:N_BLOCKS], messages[N_BLOCKS:]

    loads = []
    row = sem = 0
    for pieces, queue in zip(LOADS, LOAD_QUEUE):
        loads.append([])
        for rows, columns in pieces:
            window = (pl.ds(row, rows), pl.ds(*columns))
            copy = pltpu.make_async_copy(x_hbm.at[window], x_vmem.at[window], load_sems.at[sem])
            copy.start(priority=queue)
            loads[-1].append((copy, row, rows, columns))
            sem += 1
            if columns != LEFT:
                row += rows

    peer = lax.axis_index("x") * 2 + (1 - lax.axis_index("y"))
    barrier = pltpu.get_barrier_semaphore()
    pl.semaphore_signal(barrier, 1, device_id=peer, device_id_type=pl.DeviceIdType.LOGICAL)

    lane = lax.broadcasted_iota(jnp.int32, (SUBLANES, LANES), 1)
    group_of_lane, row_of_lane = lane >> 3, lane & (SUBLANES - 1)

    partial, sends = [], []
    for block in range(N_BLOCKS):
        left, sums = {}, {}
        for copy, row, rows, columns in loads[block]:
            copy.wait()
            for r in range(row, row + rows, SUBLANES):
                group = r % LANES // SUBLANES
                if columns != RIGHT:
                    left[group] = x_vmem[r:r + SUBLANES, :LANES]
                if columns != LEFT:
                    both = left[group] + x_vmem[r:r + SUBLANES, LANES:]
                    sums[group] = jnp.sum(both, axis=1, keepdims=True)

        merged = jnp.zeros((SUBLANES, LANES), jnp.float32)
        for group in MERGE_ORDER[block]:
            merged = jnp.where(group_of_lane == group, sums[group], merged)
        partial.append(jnp.take_along_axis(merged, row_of_lane, axis=0)[:1])

        outbox[block][...] = partial[block]
        if block == 0:
            pl.semaphore_wait(barrier, 1)
        sends.append(pltpu.make_async_remote_copy(
            outbox[block], inbox[block], send_sems.at[block], recv_sems.at[block],
            device_id=peer, device_id_type=pl.DeviceIdType.LOGICAL))
        sends[block].start()

    for block in range(N_BLOCKS):
        if block == N_BLOCKS - 1:
            for send in sends:
                send.wait_send()
        sends[block].wait_recv()
        out_ref[pl.ds(block, 1)] = partial[block] + inbox[block][...]


def pallas_dist_sum_ax1_xy_m512_n256_kernel(x: jax.Array):
    assert x.shape == SHARD_SHAPE and x.dtype == jnp.float32
    out = pl.pallas_call(
        _kernel_body,
        out_shape=jax.ShapeDtypeStruct((N_BLOCKS, LANES), jnp.float32),
        in_specs=[pl.BlockSpec(memory_space=pltpu.MemorySpace.HBM)],
        out_specs=pl.BlockSpec(memory_space=pltpu.VMEM),
        scratch_shapes=[
            pltpu.VMEM(SHARD_SHAPE, jnp.float32),
            pltpu.SemaphoreType.DMA((sum(len(pieces) for pieces in LOADS),)),
            pltpu.SemaphoreType.DMA((N_BLOCKS,)),
            pltpu.SemaphoreType.DMA((N_BLOCKS,)),
            *[pltpu.VMEM((1, LANES), jnp.float32)] * (2 * N_BLOCKS),
        ],
        compiler_params=pltpu.CompilerParams(
            collective_id=0,
            disable_bounds_checks=True,
            disable_semaphore_checks=True,
            flags={"XLA_TPU_RESCHEDULE_DMA_DONES": True},
        ),
    )(x)
    return out.reshape(SHARD_SHAPE[0], 1)
```

```python
import jax
import jax.numpy as jnp
from jax import lax
from jax.experimental import pallas as pl
from jax.experimental.pallas import tpu as pltpu

SUBLANES = 8
LANES = 128
SHARD_SHAPE = (512, 256)
N_BLOCKS = SHARD_SHAPE[0] // LANES
GROUPS_PER_BLOCK = LANES // SUBLANES

LEFT, RIGHT, BOTH = (0, LANES), (LANES, LANES), (0, 2 * LANES)

LOADS = (
    ((128, BOTH),),
    ((128, BOTH),),
    ((32, BOTH),) + 4 * ((24, BOTH),),
    2 * ((32, BOTH),) + 5 * ((8, BOTH),) + 3 * ((8, LEFT), (8, RIGHT)),
)
LOAD_QUEUE = (0, 0, 1, 1)

TAIL_GROUPS = (14, 12, 13, 15)
MESSAGES = (
    (tuple(range(GROUPS_PER_BLOCK)),),
    (tuple(range(GROUPS_PER_BLOCK)),),
    (tuple(range(GROUPS_PER_BLOCK)),),
    ((8, 0, 1, 9, 2, 3, 10, 4, 5, 11, 6, 7), TAIL_GROUPS),
)
N_MESSAGES = N_BLOCKS + 1


def _kernel_body(x_hbm, out_ref, x_vmem, load_sems, send_sems, recv_sems, *boxes):
    outbox, inbox = boxes[:N_MESSAGES], boxes[N_MESSAGES:]

    loads = []
    row = sem = 0
    for pieces, queue in zip(LOADS, LOAD_QUEUE):
        loads.append([])
        for rows, columns in pieces:
            window = (pl.ds(row, rows), pl.ds(*columns))
            copy = pltpu.make_async_copy(x_hbm.at[window], x_vmem.at[window], load_sems.at[sem])
            copy.start(priority=queue)
            loads[-1].append((copy, row, rows, columns))
            sem += 1
            if columns != LEFT:
                row += rows

    peer = lax.axis_index("x") * 2 + (1 - lax.axis_index("y"))
    barrier = pltpu.get_barrier_semaphore()
    pl.semaphore_signal(barrier, 1, device_id=peer, device_id_type=pl.DeviceIdType.LOGICAL)

    lane = lax.broadcasted_iota(jnp.int32, (SUBLANES, LANES), 1)
    group_of_lane, row_of_lane = lane >> 3, lane & (SUBLANES - 1)

    mine, sends = [], []
    for block in range(N_BLOCKS):
        left, sums = {}, {}
        for copy, row, rows, columns in loads[block]:
            copy.wait()
            for r in range(row, row + rows, SUBLANES):
                group = r % LANES // SUBLANES
                if columns != RIGHT:
                    left[group] = x_vmem[r:r + SUBLANES, :LANES]
                if columns != LEFT:
                    both = left[group] + x_vmem[r:r + SUBLANES, LANES:]
                    sums[group] = jnp.sum(both, axis=1, keepdims=True)

        for groups in MESSAGES[block]:
            merged = jnp.zeros((SUBLANES, LANES), jnp.float32)
            for group in groups:
                merged = jnp.where(group_of_lane == group, sums[group], merged)
            mine.append(jnp.take_along_axis(merged, row_of_lane, axis=0)[:1])

            i = len(sends)
            outbox[i][...] = mine[i]
            if i == 0:
                pl.semaphore_wait(barrier, 1)
            sends.append(pltpu.make_async_remote_copy(
                outbox[i], inbox[i], send_sems.at[i], recv_sems.at[i],
                device_id=peer, device_id_type=pl.DeviceIdType.LOGICAL))
            sends[i].start()

    last, tail = N_BLOCKS - 1, N_BLOCKS
    for block in range(last):
        sends[block].wait_recv()
        out_ref[pl.ds(block, 1)] = mine[block] + inbox[block][...]
    for send in sends:
        send.wait_send()

    sends[tail].wait_recv()
    lane = lax.broadcasted_iota(jnp.int32, (1, LANES), 1)
    peer_tail = jnp.zeros((1, LANES), jnp.float32)
    for j in range(min(TAIL_GROUPS) * SUBLANES, LANES):
        peer_tail = jnp.where(lane == j, inbox[tail][0, j], peer_tail)
    sends[last].wait_recv()
    out_ref[pl.ds(last, 1)] = (mine[last] + mine[tail] + inbox[last][...]) + peer_tail


def pallas_dist_sum_ax1_xy_m512_n256_kernel(x: jax.Array):
    assert x.shape == SHARD_SHAPE and x.dtype == jnp.float32
    out = pl.pallas_call(
        _kernel_body,
        out_shape=jax.ShapeDtypeStruct((N_BLOCKS, LANES), jnp.float32),
        in_specs=[pl.BlockSpec(memory_space=pltpu.MemorySpace.HBM)],
        out_specs=pl.BlockSpec(memory_space=pltpu.VMEM),
        scratch_shapes=[
            pltpu.VMEM(SHARD_SHAPE, jnp.float32),
            pltpu.SemaphoreType.DMA((sum(len(pieces) for pieces in LOADS),)),
            pltpu.SemaphoreType.DMA((N_MESSAGES,)),
            pltpu.SemaphoreType.DMA((N_MESSAGES,)),
            *[pltpu.VMEM((1, LANES), jnp.float32)] * N_MESSAGES,
            *[pltpu.VMEM((1, LANES), jnp.float32)] * N_BLOCKS,
            pltpu.SMEM((1, LANES), jnp.float32),
        ],
        compiler_params=pltpu.CompilerParams(
            collective_id=0,
            disable_bounds_checks=True,
            disable_semaphore_checks=True,
            flags={"XLA_TPU_RESCHEDULE_DMA_DONES": True},
        ),
    )(x)
    return out.reshape(SHARD_SHAPE[0], 1)
```

```python
import jax
import jax.numpy as jnp
from jax import lax
from jax.experimental import pallas as pl
from jax.experimental.pallas import tpu as pltpu

SUBLANES = 8
LANES = 128
ROWS, COLUMNS = 512, 256

WRAPPED_ROWS = 64
N_STAGES = ROWS // LANES
GROUPS_PER_STAGE = LANES // SUBLANES

PIECES = (
    ((WRAPPED_ROWS, 1), (LANES - WRAPPED_ROWS, 1)),
    ((128, 1),),
    ((32, 1),) + 4 * ((24, 1),),
    2 * ((32, 1),) + 4 * ((8, 1),) + 4 * ((8, 2),),
)
N_LOADS = sum(copies for pieces in PIECES for _, copies in pieces)
LOAD_QUEUE = (0, 0, 1, 1)

TAIL_GROUPS = (14, 12, 13, 15)
MESSAGES = (
    (tuple(range(GROUPS_PER_STAGE)),),
    (tuple(range(GROUPS_PER_STAGE)),),
    (tuple(range(GROUPS_PER_STAGE)),),
    ((8, 0, 1, 9, 2, 3, 10, 4, 5, 11, 6, 7), TAIL_GROUPS),
)
N_MESSAGES = N_STAGES + 1


def _kernel_body(x_hbm, out_ref, x_vmem, load_sems, send_sems, recv_sems, *boxes):
    outbox, inbox = boxes[:N_MESSAGES], boxes[N_MESSAGES:]

    loads = []
    row, sem = ROWS - WRAPPED_ROWS, 0
    for pieces, queue in zip(PIECES, LOAD_QUEUE):
        loads.append([])
        for rows, n_copies in pieces:
            copies, columns = [], COLUMNS // n_copies
            for i in range(n_copies):
                window = (pl.ds(row, rows), pl.ds(i * columns, columns))
                copies.append(
                    pltpu.make_async_copy(x_hbm.at[window], x_vmem.at[window], load_sems.at[sem]))
                copies[i].start(priority=queue)
                sem += 1
            loads[-1].append((copies, row, rows))
            row = (row + rows) % ROWS

    peer = lax.axis_index("x") * 2 + (1 - lax.axis_index("y"))
    barrier = pltpu.get_barrier_semaphore()
    pl.semaphore_signal(barrier, 1, device_id=peer, device_id_type=pl.DeviceIdType.LOGICAL)

    lane = lax.broadcasted_iota(jnp.int32, (SUBLANES, LANES), 1)
    group_of_lane = ((lane + WRAPPED_ROWS) & (LANES - 1)) >> 3
    row_of_lane = lane & (SUBLANES - 1)

    mine, sends = [], []
    for stage in range(N_STAGES):
        sums = []
        for copies, row, rows in loads[stage]:
            starts = range(row, row + rows, SUBLANES)
            copies[0].wait()
            lefts = [x_vmem[r:r + SUBLANES, :LANES] for r in starts]
            if len(copies) == 2:
                copies[1].wait()
            for r, left in zip(starts, lefts):
                halves = left + x_vmem[r:r + SUBLANES, LANES:]
                sums.append(jnp.sum(halves, axis=1, keepdims=True))

        for groups in MESSAGES[stage]:
            merged = jnp.zeros((SUBLANES, LANES), jnp.float32)
            for group in groups:
                merged = jnp.where(group_of_lane == group, sums[group], merged)
            mine.append(jnp.take_along_axis(merged, row_of_lane, axis=0)[:1])

            i = len(sends)
            outbox[i][...] = mine[i]
            if i == 0:
                pl.semaphore_wait(barrier, 1)
            sends.append(pltpu.make_async_remote_copy(
                outbox[i], inbox[i], send_sems.at[i], recv_sems.at[i],
                device_id=peer, device_id_type=pl.DeviceIdType.LOGICAL))
            sends[i].start()

    lane = lax.broadcasted_iota(jnp.int32, (1, LANES), 1)
    same_stage = lane < LANES - WRAPPED_ROWS
    last, tail = N_STAGES - 1, N_STAGES
    total = []
    for stage in range(last):
        sends[stage].wait_recv()
        total.append(mine[stage] + inbox[stage][...])
        if stage > 0:
            out_ref[pl.ds(stage - 1, 1)] = jnp.where(same_stage, total[stage - 1], total[stage])
    for send in sends:
        send.wait_send()

    sends[tail].wait_recv()
    peer_tail = jnp.zeros((1, LANES), jnp.float32)
    for j in range(min(TAIL_GROUPS) * SUBLANES - WRAPPED_ROWS, LANES - WRAPPED_ROWS):
        peer_tail = jnp.where(lane == j, inbox[tail][0, j], peer_tail)
    sends[last].wait_recv()
    total.append(mine[last] + mine[tail] + inbox[last][...])
    out_ref[pl.ds(last - 1, 1)] = jnp.where(same_stage, total[last - 1], total[last])
    out_ref[pl.ds(last, 1)] = jnp.where(same_stage, total[last], total[0]) + peer_tail


def pallas_dist_sum_ax1_xy_m512_n256_kernel(x: jax.Array):
    assert x.shape == (ROWS, COLUMNS) and x.dtype == jnp.float32
    out = pl.pallas_call(
        _kernel_body,
        out_shape=jax.ShapeDtypeStruct((N_STAGES, LANES), jnp.float32),
        in_specs=[pl.BlockSpec(memory_space=pltpu.MemorySpace.HBM)],
        out_specs=pl.BlockSpec(memory_space=pltpu.VMEM),
        scratch_shapes=[
            pltpu.VMEM((ROWS, COLUMNS), jnp.float32),
            pltpu.SemaphoreType.DMA((N_LOADS,)),
            pltpu.SemaphoreType.DMA((N_MESSAGES,)),
            pltpu.SemaphoreType.DMA((N_MESSAGES,)),
            *[pltpu.VMEM((1, LANES), jnp.float32)] * N_MESSAGES,
            *[pltpu.VMEM((1, LANES), jnp.float32)] * N_STAGES,
            pltpu.SMEM((1, LANES), jnp.float32),
        ],
        compiler_params=pltpu.CompilerParams(
            collective_id=0,
            disable_semaphore_checks=True,
            flags={"XLA_TPU_RESCHEDULE_DMA_DONES": True},
        ),
    )(x)
    return out.reshape(ROWS, 1)
```
